```python
import numpy as np

kernel_name = "dist_mean_ax1_xy_m4096_n1024"

def setup_inputs():
    return {"x": np.random.randn(8192, 2048).astype(np.float32)}

def reference(x: np.ndarray) -> np.ndarray:
    return np.mean(x, axis=1, keepdims=True)
```

```python
import jax
import jax.numpy as jnp
from jax import lax
from jax.experimental import pallas as pl
from jax.experimental.pallas import tpu as pltpu

LANES = 128
SUBLANES = 8
GROUP = 128

SWAPPED_ROWS = 208
BIG_CHUNK = 4
TAIL = (96, 24, 8)


def pallas_dist_mean_ax1_xy_m4096_n1024_kernel(
    x: jax.Array,
):
    m, n = x.shape
    groups = m // GROUP
    last = groups - 1
    first_bulk = 2
    n_big = (last - first_bulk - 3) // BIG_CHUNK
    first_single = first_bulk + n_big * BIG_CHUNK
    chunks = [(first_bulk + i * BIG_CHUNK, BIG_CHUNK) for i in range(n_big)]
    chunks += [(g, 1) for g in range(first_single, last)]
    scale = 1.0 / (2 * n)

    def kernel_body(
        x_ref, o_ref, rows, mine, theirs,
        chunk_sems, tail_sems, rest_sem, swap_send, swap_recv, sum_send, sum_recv,
    ):
        def load(start, size, sem):
            return pltpu.make_async_copy(
                x_ref.at[pl.ds(start, size)], rows.at[pl.ds(start, size)], sem
            )

        loads = [
            load(g * GROUP, s * GROUP, chunk_sems.at[i])
            for i, (g, s) in enumerate(chunks)
        ]
        loads[0].start()

        peer = (lax.axis_index("x"), 1 - lax.axis_index("y"))

        def to_peer(src, dst, send_sem, recv_sem):
            return pltpu.make_async_remote_copy(
                src, dst, send_sem, recv_sem,
                device_id=peer, device_id_type=pl.DeviceIdType.MESH,
            )

        barrier = pltpu.get_barrier_semaphore()
        pl.semaphore_signal(
            barrier, inc=1, device_id=peer, device_id_type=pl.DeviceIdType.MESH
        )
        loads[1].start()
        pl.semaphore_wait(barrier, 1)

        swaps = [
            to_peer(
                x_ref.at[pl.ds(start, size)], rows.at[pl.ds(start, size)],
                swap_send.at[i], swap_recv.at[i],
            )
            for i, (start, size) in enumerate(
                [(0, GROUP), (GROUP, SWAPPED_ROWS - GROUP)]
            )
        ]
        for swap in swaps:
            swap.start()
        rest = load(SWAPPED_ROWS, first_bulk * GROUP - SWAPPED_ROWS, rest_sem)
        rest.start()
        for copy in loads[2:]:
            copy.start()
        tail = []
        start = last * GROUP
        for i, size in enumerate(TAIL):
            tail.append((start, size, load(start, size, tail_sems.at[i])))
            start += size
        for _, _, copy in tail:
            copy.start()

        shape = (SUBLANES, LANES)
        diagonal = lax.broadcasted_iota(jnp.int32, shape, 1) - lax.broadcasted_iota(
            jnp.int32, shape, 0
        )
        zeros = jnp.zeros(shape, jnp.float32)

        def fold(start, size):
            folded = []
            for k in range(size // SUBLANES):
                r = start + k * SUBLANES
                if not isinstance(r, int):
                    r = pl.multiple_of(r, SUBLANES)
                parts = [
                    rows[pl.ds(r, SUBLANES), pl.ds(j * LANES, LANES)]
                    for j in range(n // LANES)
                ]
                while len(parts) > 1:
                    parts = [a + b for a, b in zip(parts[::2], parts[1::2])]
                folded.append(parts[0])
            return folded

        def spread(folded, lane, acc):
            for k, tile in enumerate(folded):
                sums = jnp.sum(tile, axis=1, keepdims=True)
                acc = jnp.where(diagonal == lane + k * SUBLANES, sums, acc)
            return acc

        def reduce_group(g):
            acc = spread(fold(g * GROUP, GROUP), 0, zeros)
            mine[pl.ds(g, 1), :] = jnp.sum(acc, axis=0, keepdims=True)

        def bulk_step(g, carry):
            k = g - first_bulk

            @pl.when(jnp.logical_and(g < first_single, lax.rem(k, BIG_CHUNK) == 0))
            def _():
                load(0, BIG_CHUNK * GROUP, chunk_sems.at[lax.div(k, BIG_CHUNK)]).wait()

            @pl.when(g >= first_single)
            def _():
                index = jnp.maximum(n_big + g - first_single, 0)
                load(0, GROUP, chunk_sems.at[index]).wait()

            reduce_group(g)
            return carry

        sends = []

        def send(g0, size):
            i = len(sends)
            copy = to_peer(
                mine.at[pl.ds(g0, size)], theirs.at[pl.ds(g0, size)],
                sum_send.at[i], sum_recv.at[i],
            )
            copy.start()
            sends.append(copy)

        lax.fori_loop(first_bulk, 20, bulk_step, 0)
        swaps[0].wait_recv()
        reduce_group(0)
        send(0, 1)
        lax.fori_loop(20, last - 3, bulk_step, 0)
        send(first_bulk, last - 3 - first_bulk)
        lax.fori_loop(last - 3, last - 1, bulk_step, 0)
        rest.wait()
        swaps[1].wait_recv()
        reduce_group(1)
        send(1, 1)
        lax.fori_loop(last - 1, last, bulk_step, 0)
        send(last - 3, 3)

        start, size, copy = tail[0]
        copy.wait()
        acc = spread(fold(start, size), 0, zeros)
        folded = []
        for start, size, copy in tail[1:]:
            copy.wait()
            folded += fold(start, size)
        acc = spread(folded, TAIL[0], acc)
        mine[pl.ds(last, 1), :] = jnp.sum(acc, axis=0, keepdims=True)
        send(last, 1)

        for swap in swaps:
            swap.wait_send()
        for copy in sends[:-1]:
            copy.wait()
        head = pl.ds(0, groups - SUBLANES)
        o_ref[head, :] = (mine[head, :] + theirs[head, :]) * scale
        sends[-1].wait()
        end = pl.ds(groups - SUBLANES, SUBLANES)
        o_ref[end, :] = (mine[end, :] + theirs[end, :]) * scale

    out = pl.pallas_call(
        kernel_body,
        in_specs=[pl.BlockSpec(memory_space=pltpu.HBM)],
        out_specs=pl.BlockSpec(memory_space=pltpu.VMEM),
        out_shape=pltpu.VMEM((groups, LANES), jnp.float32),
        scratch_shapes=[
            pltpu.VMEM((m, n), jnp.float32),
            pltpu.VMEM((groups, LANES), jnp.float32),
            pltpu.VMEM((groups, LANES), jnp.float32),
            pltpu.SemaphoreType.DMA((len(chunks),)),
            pltpu.SemaphoreType.DMA((len(TAIL),)),
            pltpu.SemaphoreType.DMA,
            pltpu.SemaphoreType.DMA((2,)),
            pltpu.SemaphoreType.DMA((2,)),
            pltpu.SemaphoreType.DMA((5,)),
            pltpu.SemaphoreType.DMA((5,)),
        ],
        compiler_params=pltpu.CompilerParams(
            vmem_limit_bytes=32 * 1024 * 1024,
            collective_id=0,
            disable_bounds_checks=True,
            disable_semaphore_checks=True,
        ),
    )(x)
    return out.reshape(m, 1)
```

```python
import jax
import jax.numpy as jnp
from jax import lax
from jax.experimental import pallas as pl
from jax.experimental.pallas import tpu as pltpu

LANES = 128
SUBLANES = 8
GROUP = LANES

Y_GROUP, Y_ROWS = 0, 216
X_GROUP, X_ROWS = 2, 208
SMEM_GROUP, SMEM_ROWS = 4, 112
FIRST_BULK = 5

BIG_CHUNK = 4
N_SINGLE = 6
TAIL = (96, 24, 8)


def pallas_dist_mean_ax1_xy_m4096_n1024_kernel(
    x: jax.Array,
):
    m, n = x.shape
    groups = m // GROUP
    last = groups - 1
    first_single = last - N_SINGLE
    n_big = (first_single - FIRST_BULK) // BIG_CHUNK
    assert first_single == FIRST_BULK + n_big * BIG_CHUNK
    scale = 1.0 / (2 * n)

    def kernel_body(
        x_ref,
        o_ref,
        rows,
        staged,
        mine,
        theirs,
        x_out,
        x_in,
        last_out,
        last_in,
        big_sems,
        single_sems,
        tail_sems,
        rest_sems,
        staged_sems,
        row_send,
        row_recv,
        sum_send,
        sum_recv,
        diagonal_entered,
    ):
        def load(start, size, sem):
            return pltpu.make_async_copy(
                x_ref.at[pl.ds(start, size)], rows.at[pl.ds(start, size)], sem
            )

        def load_big(i):
            start = (FIRST_BULK + i * BIG_CHUNK) * GROUP
            return load(aligned(start, GROUP), BIG_CHUNK * GROUP, big_sems.at[i])

        def load_single(i):
            start = (first_single + i) * GROUP
            return load(aligned(start, GROUP), GROUP, single_sems.at[i])

        load_big(0).start()
        staged_rows = pl.ds(SMEM_GROUP * GROUP, SMEM_ROWS)
        stage = pltpu.make_async_copy(x_ref.at[staged_rows], staged, staged_sems.at[0])
        unstage = pltpu.make_async_copy(staged, rows.at[staged_rows], staged_sems.at[1])
        stage.start()

        my_x, my_y = lax.axis_index("x"), lax.axis_index("y")
        y_peer = (my_x, 1 - my_y)
        x_peer = (1 - my_x, my_y)
        diagonal_peer = (1 - my_x, 1 - my_y)

        def signal(sem, device):
            pl.semaphore_signal(
                sem, inc=1, device_id=device, device_id_type=pl.DeviceIdType.MESH
            )

        barrier = pltpu.get_barrier_semaphore()
        signal(barrier, y_peer)
        signal(barrier, x_peer)

        rests = [
            load(group * GROUP + size, -size % GROUP, rest_sems.at[i])
            for i, (group, size) in enumerate(
                [(Y_GROUP, Y_ROWS), (X_GROUP, X_ROWS), (SMEM_GROUP, SMEM_ROWS)]
            )
        ]
        for copy in rests:
            copy.start()
        for i in range(1, n_big):
            load_big(i).start()
        for i in range(N_SINGLE):
            load_single(i).start()
        tail = []
        for i, size in enumerate(TAIL):
            start = last * GROUP + sum(TAIL[:i])
            tail.append((start, size, load(start, size, tail_sems.at[i])))
            tail[-1][2].start()

        pl.semaphore_wait(barrier, 2)

        def remote(src, dst, send_sem, recv_sem, device):
            return pltpu.make_async_remote_copy(
                src,
                dst,
                send_sem,
                recv_sem,
                device_id=device,
                device_id_type=pl.DeviceIdType.MESH,
            )

        swaps = []

        def swap_rows(start, size, device):
            span, i = pl.ds(start, size), len(swaps)
            copy = remote(
                x_ref.at[span], rows.at[span], row_send.at[i], row_recv.at[i], device
            )
            copy.start()
            swaps.append(copy)
            return copy

        y_first = swap_rows(Y_GROUP * GROUP, GROUP, y_peer)
        x_first = swap_rows(X_GROUP * GROUP, GROUP, x_peer)
        y_second = swap_rows((Y_GROUP + 1) * GROUP, Y_ROWS - GROUP, y_peer)
        x_second = swap_rows((X_GROUP + 1) * GROUP, X_ROWS - GROUP, x_peer)
        signal(diagonal_entered, x_peer)

        messages = []

        def send(src, dst, device):
            i = len(messages)
            copy = remote(src, dst, sum_send.at[i], sum_recv.at[i], device)
            copy.start()
            messages.append(copy)

        def share(group, size):
            span = pl.ds(group, size)
            send(mine.at[span], theirs.at[span], y_peer)

        tile = (SUBLANES, LANES)
        lane = lax.broadcasted_iota(jnp.int32, tile, 1)
        diagonal = lane - lax.broadcasted_iota(jnp.int32, tile, 0)

        def fold(start, size):
            folded = []
            for k in range(size // SUBLANES):
                span = pl.ds(aligned(start + k * SUBLANES, SUBLANES), SUBLANES)
                parts = [rows[span, pl.ds(j, LANES)] for j in range(0, n, LANES)]
                while len(parts) > 1:
                    parts = [a + b for a, b in zip(parts[::2], parts[1::2])]
                folded.append(parts[0])
            return folded

        def row_sums(folded, first_lane=0):
            sums = jnp.zeros(tile, jnp.float32)
            for k, part in enumerate(folded):
                sums = jnp.where(
                    diagonal == first_lane + k * SUBLANES,
                    jnp.sum(part, axis=1, keepdims=True),
                    sums,
                )
            return jnp.sum(sums, axis=0, keepdims=True)

        def reduce_group(group):
            mine[pl.ds(group, 1), :] = row_sums(fold(group * GROUP, GROUP))

        def reduce_bulk(begin, end):
            @pl.loop(begin, end)
            def _(group):
                if end <= first_single:
                    index = group - FIRST_BULK

                    @pl.when(lax.rem(index, BIG_CHUNK) == 0)
                    def _():
                        load_big(lax.div(index, BIG_CHUNK)).wait()
                else:
                    load_single(group - first_single).wait()
                reduce_group(group)

        def reduce_y_rows(i, swap):
            swap.wait_recv()
            reduce_group(Y_GROUP + i)
            share(Y_GROUP + i, 1)

        def reduce_x_rows(i, swap, size):
            swap.wait_recv()
            group = X_GROUP + i
            sums = row_sums(fold(group * GROUP, GROUP))
            foreign = lane[:1] < size
            x_out[pl.ds(i, 1), :] = jnp.where(foreign, sums, 0.0)
            mine[pl.ds(group, 1), :] = jnp.where(foreign, 0.0, sums)
            for j, device in enumerate((diagonal_peer, x_peer)):
                send(x_out.at[pl.ds(i, 1)], x_in.at[j, pl.ds(i, 1)], device)
            share(group, 1)

        reduce_bulk(FIRST_BULK, 14)
        stage.wait()
        unstage.start()
        for copy in rests:
            copy.wait()
        pl.semaphore_wait(diagonal_entered, 1)
        reduce_bulk(14, first_single)
        reduce_y_rows(0, y_first)
        reduce_x_rows(0, x_first, GROUP)
        reduce_bulk(first_single, last - 3)
        reduce_x_rows(1, x_second, X_ROWS - GROUP)
        share(FIRST_BULK, last - 3 - FIRST_BULK)
        reduce_bulk(last - 3, last - 2)
        unstage.wait()
        reduce_group(SMEM_GROUP)
        share(SMEM_GROUP, 1)
        reduce_bulk(last - 2, last)
        reduce_y_rows(1, y_second)
        share(last - 3, 3)

        start, size, copy = tail[0]
        copy.wait()
        last_row = pl.ds(last, 1)
        mine[last_row, :] = row_sums(fold(start, size))
        share(last, 1)
        folded = []
        for start, size, copy in tail[1:]:
            copy.wait()
            folded += fold(start, size)
        last_sums = row_sums(folded, TAIL[0])
        last_out[...] = last_sums
        send(last_out, last_in, y_peer)

        for swap in swaps:
            swap.wait_send()
        for copy in messages[:-1]:
            copy.wait()
        for i in range(2):
            span = pl.ds(i, 1)
            theirs[pl.ds(X_GROUP + i, 1), :] += x_in[0, span, :] + x_in[1, span, :]
        o_ref[...] = (mine[...] + theirs[...]) * scale
        total = mine[last_row, :] + theirs[last_row, :] + last_sums
        messages[-1].wait()
        arrived = [jnp.zeros((1, LANES), jnp.float32)] * 2
        for i in range(TAIL[0], LANES):
            arrived[i % 2] = jnp.where(lane[:1] == i, last_in[0, i], arrived[i % 2])
        o_ref[last_row, :] = (total + arrived[0] + arrived[1]) * scale

    f32 = jnp.float32
    dma = pltpu.SemaphoreType.DMA
    n_messages = 13
    out = pl.pallas_call(
        kernel_body,
        in_specs=[pl.BlockSpec(memory_space=pltpu.HBM)],
        out_specs=pl.BlockSpec(memory_space=pltpu.VMEM),
        out_shape=jax.ShapeDtypeStruct((groups, LANES), f32),
        scratch_shapes=[
            pltpu.VMEM((m, n), f32),
            pltpu.SMEM((SMEM_ROWS, n), f32),
            pltpu.VMEM((groups, LANES), f32),
            pltpu.VMEM((groups, LANES), f32),
            pltpu.VMEM((SUBLANES, LANES), f32),
            pltpu.VMEM((2, SUBLANES, LANES), f32),
            pltpu.VMEM((1, LANES), f32),
            pltpu.SMEM((1, LANES), f32),
            dma((n_big,)),
            dma((N_SINGLE,)),
            dma((len(TAIL),)),
            dma((3,)),
            dma((2,)),
            dma((4,)),
            dma((4,)),
            dma((n_messages,)),
            dma((n_messages,)),
            pltpu.SemaphoreType.REGULAR,
        ],
        compiler_params=pltpu.CompilerParams(
            vmem_limit_bytes=32 * 1024 * 1024,
            collective_id=0,
            disable_bounds_checks=True,
            disable_semaphore_checks=True,
        ),
    )(x)
    return out.reshape(m, 1)


def aligned(index, multiple):
    return index if isinstance(index, int) else pl.multiple_of(index, multiple)
```
